```python
import numpy as np

kernel_name = "dist_rope_attn_qseq_b2_sq128_d512_hq4_dh64"

def setup_inputs():
    x = np.random.randn(2, 512, 512).astype(np.float32)
    Wq = np.random.randn(512, 256).astype(np.float32) * 0.02
    Wk = np.random.randn(512, 256).astype(np.float32) * 0.02
    Wv = np.random.randn(512, 256).astype(np.float32) * 0.02
    Wo = np.random.randn(256, 512).astype(np.float32) * 0.02
    return {"x": x, "Wq": Wq, "Wk": Wk, "Wv": Wv, "Wo": Wo}

def reference(x, Wq, Wk, Wv, Wo):
    B, Sq, Hq, Dh = 2, 512, 4, 64
    inv = 1.0 / (10000.0 ** (np.arange(0, Dh, 2) / Dh))
    pos = np.arange(Sq)[:, None] * inv[None, :]
    cos = np.repeat(np.cos(pos), 2, axis=-1).astype(np.float32)
    sin = np.repeat(np.sin(pos), 2, axis=-1).astype(np.float32)
    def rot(t):
        t2 = t.reshape(B, Sq, Hq, Dh // 2, 2)
        t_r = np.stack([-t2[..., 1], t2[..., 0]], axis=-1).reshape(B, Sq, Hq, Dh)
        return t * cos[None, :, None, :] + t_r * sin[None, :, None, :]
    Q = rot((x @ Wq).reshape(B, Sq, Hq, Dh))
    K = rot((x @ Wk).reshape(B, Sq, Hq, Dh))
    V = (x @ Wv).reshape(B, Sq, Hq, Dh)
    s = np.einsum('bihd,bjhd->bhij', Q, K).astype(np.float32) * 0.125
    s_max = s.max(axis=-1, keepdims=True)
    w = np.exp(s - s_max)
    w = w / w.sum(axis=-1, keepdims=True)
    ctx = np.einsum('bhij,bjhd->bihd', w, V).reshape(B, Sq, Hq * Dh)
    return ctx @ Wo
```

```python
import functools
import numpy as np
import jax
import jax.numpy as jnp
from jax import lax
from jax.experimental import pallas as pl
from jax.experimental.pallas import tpu as pltpu

f32 = jnp.float32
bf16 = jnp.bfloat16
NT = (((1,), (1,)), ((), ()))
TN = (((0,), (0,)), ((), ()))
MESH = pl.DeviceIdType.MESH

R = 128
DM = 512
HD = 256
H = 4
D = 64
QSCALE = float(0.125 * np.log2(np.e))
LN_BASE = float(np.log(10000.0))


def _dot(a, b, dims=None):
    if dims is None:
        return jnp.dot(a, b, preferred_element_type=f32)
    return lax.dot_general(a, b, dims, preferred_element_type=f32)


def make_kernel(xchunks=2):
    CR = R // xchunks

    def body(x_hbm, wq_hbm, wk_hbm, wv_hbm, wo_hbm, out_ref,
             xf, wq32, wk32, wv32, wo32,
             xb, xr, wqb, wkb, wvT, wob,
             qT_own, qT_rem, kbuf, vT,
             o_own, st_own, o_send, st_send, o_recv, st_recv, ctxT,
             tabs,
             ld_sem, xs_sem, xr_sem, qs_sem, qr_sem, os_sem, or_sem, ss_sem, sr_sem):
        me = lax.axis_index("i")
        pa = jnp.bitwise_xor(me, 1)
        pb = 3 - me
        kv_partner = (pa, pb)
        q_partner = (pb, pa)

        x_ld = {}
        n = 0
        for c in range(xchunks):
            for b in range(2):
                x_ld[b, c] = pltpu.make_async_copy(
                    x_hbm.at[b, pl.ds(c * CR, CR)], xf.at[b, pl.ds(c * CR, CR)], ld_sem.at[n])
                x_ld[b, c].start()
                n += 1
        w_ld = []
        for src, dst in ((wq_hbm, wq32), (wk_hbm, wk32), (wv_hbm, wv32), (wo_hbm, wo32)):
            cp = pltpu.make_async_copy(src, dst, ld_sem.at[n])
            cp.start()
            w_ld.append(cp)
            n += 1

        bar = pltpu.get_barrier_semaphore()
        pl.semaphore_signal(bar, inc=1, device_id=(pa,), device_id_type=MESH)
        pl.semaphore_signal(bar, inc=1, device_id=(pb,), device_id_type=MESH)

        row = lax.broadcasted_iota(jnp.int32, (R, 128), 0)
        lane = lax.broadcasted_iota(jnp.int32, (R, 128), 1)
        even = (lane % 2) == 0
        inv = jnp.exp(((lane % D) // 2).astype(f32) * (-2.0 / D * LN_BASE))
        sgn = jnp.where(even, -1.0, 1.0).astype(f32)
        ang = (row + me * R).astype(f32) * inv
        c_own = jnp.cos(ang)
        s_own = jnp.sin(ang)
        tabs[0] = c_own
        tabs[1] = s_own * sgn
        tabs[2] = c_own * QSCALE
        tabs[3] = s_own * sgn * QSCALE
        inv1 = inv[0:8]
        for b in range(2):
            dang = ((kv_partner[b] - me) * R).astype(f32) * inv1
            cd = jnp.cos(dang)[0:1]
            sd = jnp.sin(dang)[0:1]
            tabs[4 + 2 * b] = c_own * cd - s_own * sd
            tabs[5 + 2 * b] = (s_own * cd + c_own * sd) * sgn

        z = jnp.zeros((D, 128), bf16)
        for buf in (qT_own, qT_rem):
            for b in range(2):
                for h in range(H):
                    off = h * 128 + (1 - h % 2) * D
                    buf[b, off:off + D, :] = z

        def rope(t, c, s):
            ev = (lax.broadcasted_iota(jnp.int32, t.shape, 1) % 2) == 0
            sw = jnp.where(ev, pltpu.roll(t, 127, 1), pltpu.roll(t, 1, 1))
            return t * c + sw * s

        def x_send(b, c):
            return pltpu.make_async_remote_copy(
                xb.at[b, pl.ds(c * CR, CR)], xr.at[b, pl.ds(c * CR, CR)],
                xs_sem.at[b, c], xr_sem.at[b, c], device_id=(kv_partner[b],), device_id_type=MESH)

        def q_rows(h):
            return pl.ds(h * 128 + (h % 2) * D, D)

        def q_send(b, h):
            return pltpu.make_async_remote_copy(
                qT_own.at[b, q_rows(h)], qT_rem.at[b, q_rows(h)],
                qs_sem.at[b, h], qr_sem.at[b, h], device_id=(q_partner[b],), device_id_type=MESH)

        def o_send_cp(b, h):
            return pltpu.make_async_remote_copy(
                o_send.at[b, pl.ds(h * D, D)], o_recv.at[b, pl.ds(h * D, D)],
                os_sem.at[b, h], or_sem.at[b, h], device_id=(q_partner[b],), device_id_type=MESH)

        def s_send_cp(b, h):
            return pltpu.make_async_remote_copy(
                st_send.at[b, h], st_recv.at[b, h],
                ss_sem.at[b, h], sr_sem.at[b, h], device_id=(q_partner[b],), device_id_type=MESH)

        first = True
        for c in range(xchunks):
            for b in range(2):
                x_ld[b, c].wait()
                xb[b, c * CR:(c + 1) * CR, :] = xf[b, c * CR:(c + 1) * CR, :].astype(bf16)
                if first:
                    pl.semaphore_wait(bar, 2)
                    first = False
                x_send(b, c).start()

        w_ld[0].wait()
        wqb[...] = wq32[...].astype(bf16)
        eye = (lax.broadcasted_iota(jnp.int32, (128, 128), 0)
               == lax.broadcasted_iota(jnp.int32, (128, 128), 1)).astype(bf16)
        for b in (1, 0):
            q = _dot(xb[b], wqb[...])
            for t in range(2):
                qt = rope(q[:, t * 128:(t + 1) * 128], tabs[2], tabs[3]).astype(bf16)
                qtT = _dot(eye, qt, NT).astype(bf16)
                for hh in range(2):
                    h = 2 * t + hh
                    qT_own[b, h * 128 + hh * D:h * 128 + hh * D + D, :] = qtT[hh * D:(hh + 1) * D]
        for h in range(H):
            for b in (1, 0):
                q_send(b, h).start()

        def kproj(b, src, r0, nr, dst0, ct, st):
            k = _dot(src[b, r0:r0 + nr, :], wkb[...])
            for t in range(2):
                kt = rope(k[:, t * 128:(t + 1) * 128], tabs[ct, r0:r0 + nr, :], tabs[st, r0:r0 + nr, :])
                kbuf[b, dst0 + r0:dst0 + r0 + nr, t * 128:(t + 1) * 128] = kt.astype(bf16)

        def vproj(b, src, dst0):
            v = _dot(wvT[...], src[b], NT)
            vT[b, :, dst0:dst0 + R] = v.astype(bf16)

        w_ld[1].wait()
        wkb[...] = wk32[...].astype(bf16)
        for b in range(2):
            kproj(b, xb, 0, R, 0, 0, 1)
        w_ld[2].wait()
        wvT[...] = wv32[...].T.astype(bf16)
        for b in range(2):
            vproj(b, xb, 0)
        for c in range(xchunks):
            for b in range(2):
                x_send(b, c).wait_recv()
        for b in range(2):
            kproj(b, xr, 0, R, R, 4 + 2 * b, 5 + 2 * b)
            vproj(b, xr, R)

        def attn(b, h, qbuf):
            t = h // 2
            sT = _dot(kbuf[b, :, t * 128:(t + 1) * 128], qbuf[b, h * 128:(h + 1) * 128, :])
            m = jnp.max(sT, axis=0, keepdims=True)
            p = jnp.exp2(sT - m)
            l = jnp.sum(p, axis=0, keepdims=True)
            oT = _dot(vT[b, h * D:(h + 1) * D, :], p.astype(bf16))
            return oT, m, l

        for h in range(H):
            for b in (1, 0):
                q_send(b, h).wait_recv()
                oT, m, l = attn(b, h, qT_rem)
                o_send[b, h * D:(h + 1) * D, :] = oT.astype(bf16)
                st_send[b, h, 0:1, :] = m
                st_send[b, h, 1:2, :] = l
                st_send[b, h, 2:8, :] = jnp.zeros((6, 128), f32)
                o_send_cp(b, h).start()
                s_send_cp(b, h).start()

        for b in range(2):
            for h in range(H):
                oT, m, l = attn(b, h, qT_own)
                o_own[b, h * D:(h + 1) * D, :] = oT
                st_own[b, h, 0:1, :] = m
                st_own[b, h, 1:2, :] = l

        w_ld[3].wait()
        wob[...] = wo32[...].astype(bf16)

        for h in range(H):
            for b in (1, 0):
                o_send_cp(b, h).wait_recv()
                s_send_cp(b, h).wait_recv()
                m1 = st_own[b, h, 0:1, :]
                l1 = st_own[b, h, 1:2, :]
                m2 = st_recv[b, h, 0:1, :]
                l2 = st_recv[b, h, 1:2, :]
                m = jnp.maximum(m1, m2)
                a1 = jnp.exp2(m1 - m)
                a2 = jnp.exp2(m2 - m)
                inv_l = 1.0 / (a1 * l1 + a2 * l2)
                c = o_own[b, h * D:(h + 1) * D, :] * (a1 * inv_l) + \
                    o_recv[b, h * D:(h + 1) * D, :].astype(f32) * (a2 * inv_l)
                ctxT[b, h * D:(h + 1) * D, :] = c.astype(bf16)
        for b in (1, 0):
            out_ref[b] = _dot(ctxT[b], wob[...], TN)

        for c in range(xchunks):
            for b in range(2):
                x_send(b, c).wait_send()
        for h in range(H):
            for b in range(2):
                q_send(b, h).wait_send()
                o_send_cp(b, h).wait_send()
                s_send_cp(b, h).wait_send()

    return body


def kernel(x, Wq, Wk, Wv, Wo, xchunks=2):
    V = pltpu.VMEM
    DMA = pltpu.SemaphoreType.DMA
    scratch = [
        V((2, R, DM), f32), V((DM, HD), f32), V((DM, HD), f32), V((DM, HD), f32), V((HD, DM), f32),
        V((2, R, DM), bf16), V((2, R, DM), bf16), V((DM, HD), bf16), V((DM, HD), bf16), V((HD, DM), bf16), V((HD, DM), bf16),
        V((2, 512, 128), bf16), V((2, 512, 128), bf16), V((2, 2 * R, HD), bf16), V((2, HD, 2 * R), bf16),
        V((2, HD, R), f32), V((2, H, 8, 128), f32), V((2, HD, R), bf16), V((2, H, 8, 128), f32),
        V((2, HD, R), bf16), V((2, H, 8, 128), f32), V((2, HD, R), bf16),
        V((8, R, 128), f32),
        DMA((2 * xchunks + 4,)), DMA((2, xchunks)), DMA((2, xchunks)),
        DMA((2, H)), DMA((2, H)), DMA((2, H)), DMA((2, H)), DMA((2, H)), DMA((2, H)),
    ]
    return pl.pallas_call(
        make_kernel(xchunks),
        out_shape=jax.ShapeDtypeStruct((2, R, DM), f32),
        in_specs=[pl.BlockSpec(memory_space=pl.ANY)] * 5,
        out_specs=pl.BlockSpec(memory_space=pltpu.VMEM),
        scratch_shapes=scratch,
        compiler_params=pltpu.CompilerParams(collective_id=0, vmem_limit_bytes=64 * 1024 * 1024),
    )(x, Wq, Wk, Wv, Wo)


def pallas_dist_rope_attn_qseq_b2_sq128_d512_hq4_dh64_kernel(
    x: jax.Array,
    Wq: jax.Array,
    Wk: jax.Array,
    Wv: jax.Array,
    Wo: jax.Array,
):
    return kernel(x, Wq, Wk, Wv, Wo)
```

```python
import functools
import numpy as np
import jax
import jax.numpy as jnp
from jax import lax
from jax.experimental import pallas as pl
from jax.experimental.pallas import tpu as pltpu

f32 = jnp.float32
bf16 = jnp.bfloat16
NT = (((1,), (1,)), ((), ()))
TN = (((0,), (0,)), ((), ()))
MESH = pl.DeviceIdType.MESH

R = 128
DM = 512
HD = 256
H = 4
D = 64
QSCALE = float(0.125 * np.log2(np.e))
LN_BASE = float(np.log(10000.0))
OROWS = 34


XCH_DEFAULT = ((0, 1, 0, 64), (0, 1, 64, 64), (1, 2, 0, 128), (3, 1, 0, 128))


def _dot(a, b, dims=None):
    if dims is None:
        return jnp.dot(a, b, preferred_element_type=f32)
    return lax.dot_general(a, b, dims, preferred_element_type=f32)


def make_kernel(cfg):
    SS = cfg.get("ss", 4)
    SP = cfg.get("sp", 2)
    DECOUPLE = cfg.get("decouple", True)
    XCH = cfg.get("xch", XCH_DEFAULT)
    NLATE = cfg.get("nlate", 1)
    GROUPS = cfg.get("groups", ((0, 1), (2, 3), (4, 5), (6, 7)))
    ODD_FUSE = cfg.get("odd_fuse", True)
    TAB_EARLY = cfg.get("tab_early", True)
    ROPE_GATHER = cfg.get("rope_gather", True)
    XORD = cfg.get("xord", (0, 1))
    ODD_GROUPS = cfg.get("odd_groups", ((0,), (1, 2), (3, 4), (5, 6), (7,)))
    ODD_LATE_S_FIRST = cfg.get("odd_late_s_first", False)
    EVEN_GROUPS = cfg.get("even_groups", ((0, 1), (2, 3), (4, 5), (6, 7)))
    EVEN_JOINT = cfg.get("even_joint", True)
    ASYM = cfg.get("asym", True)
    MSK = cfg.get("msk", {1: 2, 2: 1, 3: 2})
    MSV = cfg.get("msv", {1: 4, 2: 2, 3: 4})

    def body(x_hbm, wq_hbm, wk_hbm, wv_hbm, wo_hbm, out_ref,
             xf, wq32, wk32, wv32, wo32,
             xb, xr, wqb, wkb, wvT, wob,
             qT_own, qT_rem, kbuf, vT,
             o_own, st_own, o_send, o_recv, ctxT,
             kpart, vpart,
             tabs,
             ld_sem, xs_sem, xr_sem, qs_sem, qr_sem, os_sem, or_sem, hs_sem):
        me = lax.axis_index("i")
        pa = jnp.bitwise_xor(me, 1)
        pb = 3 - me
        is_odd = (me % 2) == 1

        def kv_partner(b):
            return jnp.where(b == 0, pa, pb) if not isinstance(b, int) else (pa, pb)[b]

        def q_partner(b):
            return jnp.where(b == 0, pb, pa) if not isinstance(b, int) else (pb, pa)[b]

        x_ld = {}
        n = 0
        for c, (q0, nq, r0, nr) in enumerate(XCH):
            for b in XORD:
                x_ld[b, c] = pltpu.make_async_copy(
                    x_hbm.at[b, pl.ds(r0, nr), pl.ds(q0 * 128, nq * 128)],
                    xf.at[b, pl.ds(r0, nr), pl.ds(q0 * 128, nq * 128)], ld_sem.at[n])
                x_ld[b, c].start()
                n += 1

        bar = pltpu.get_barrier_semaphore()
        if ASYM:
            @pl.when(me != 2)
            def _():
                pl.semaphore_signal(bar, inc=1, device_id=(pa,), device_id_type=MESH)
                pl.semaphore_signal(bar, inc=1, device_id=(pb,), device_id_type=MESH)
        else:
            pl.semaphore_signal(bar, inc=1, device_id=(pa,), device_id_type=MESH)
            pl.semaphore_signal(bar, inc=1, device_id=(pb,), device_id_type=MESH)

        w_ld = []
        for src, dst in ((wq_hbm, wq32), (wk_hbm, wk32), (wv_hbm, wv32), (wo_hbm, wo32)):
            cp = pltpu.make_async_copy(src, dst, ld_sem.at[n])
            cp.start()
            w_ld.append(cp)
            n += 1

        if ASYM:
            @pl.when(me == 2)
            def _():
                pl.semaphore_wait(bar, 2)
                pl.semaphore_signal(hs_sem, inc=1, device_id=(pa,), device_id_type=MESH)
                pl.semaphore_signal(hs_sem, inc=1, device_id=(pb,), device_id_type=MESH)

        r16 = lax.broadcasted_iota(jnp.int32, (16, 128), 0)
        l16 = lax.broadcasted_iota(jnp.int32, (16, 128), 1)
        inv16 = jnp.exp(((l16 % D) // 2).astype(f32) * (-2.0 / D * LN_BASE))
        pos16 = jnp.where(r16 < 8, r16 + me * R,
                jnp.where(r16 == 8, 8,
                jnp.where(r16 == 9, 16,
                jnp.where(r16 == 10, 32,
                jnp.where(r16 == 11, 64,
                jnp.where(r16 == 12, (pa - me) * R, (pb - me) * R))))))
        ang16 = pos16.astype(f32) * inv16
        c16 = jnp.cos(ang16)
        s16 = jnp.sin(ang16)

        def rot(c, s, row):
            cd = c16[row:row + 1]
            sd = s16[row:row + 1]
            return c * cd - s * sd, s * cd + c * sd

        c_own, s_own = c16[0:8], s16[0:8]
        for k in range(4):
            c2, s2 = rot(c_own, s_own, 8 + k)
            c_own = jnp.concatenate([c_own, c2], axis=0)
            s_own = jnp.concatenate([s_own, s2], axis=0)
        lane = lax.broadcasted_iota(jnp.int32, (R, 128), 1)
        sgn = jnp.where((lane % 2) == 0, -1.0, 1.0).astype(f32)

        def tables_rest():
            tabs[0] = c_own
            tabs[1] = s_own * sgn
            tabs[2] = c_own * QSCALE
            tabs[3] = s_own * sgn * QSCALE
            for b in range(2):
                cb, sb = rot(c_own, s_own, 12 + b)
                tabs[4 + 2 * b] = cb
                tabs[5 + 2 * b] = sb * sgn

        if TAB_EARLY:
            tables_rest()

        def x_send(b, c):
            q0, nq, r0, nr = XCH[c]
            return pltpu.make_async_remote_copy(
                xb.at[b, pl.ds(q0, nq), pl.ds(r0, nr)], xr.at[b, pl.ds(q0, nq), pl.ds(r0, nr)],
                xs_sem.at[b, c], xr_sem.at[b, c], device_id=(kv_partner(b),), device_id_type=MESH)

        def q_send(b, h):
            rows = pl.ds(pl.multiple_of((h % 2) * D, D), D) if not isinstance(h, int) else pl.ds((h % 2) * D, D)
            return pltpu.make_async_remote_copy(
                qT_own.at[b, h, rows], qT_rem.at[b, h, rows],
                qs_sem.at[b, h], qr_sem.at[b, h], device_id=(q_partner(b),), device_id_type=MESH)

        def o_send_cp(b, h):
            return pltpu.make_async_remote_copy(
                o_send.at[b, h, pl.ds(0, OROWS)], o_recv.at[b, h, pl.ds(0, OROWS)],
                os_sem.at[b, h], or_sem.at[b, h], device_id=(q_partner(b),), device_id_type=MESH)

        b_l = jnp.where(me == 1, 1, 0)
        b_e = 1 - b_l
        first = True
        for c, (q0, nq, r0, nr) in enumerate(XCH):
            for b in XORD:
                x_ld[b, c].wait()
                for q in range(q0, q0 + nq):
                    xb[b, q, r0:r0 + nr, :] = xf[b, r0:r0 + nr, q * 128:(q + 1) * 128].astype(bf16)
                if not ASYM:
                    if first:
                        pl.semaphore_wait(bar, 2)
                        first = False
                    x_send(b, c).start()
                else:
                    if first:
                        @pl.when(me == 0)
                        def _():
                            pl.semaphore_wait(bar, 2)

                        @pl.when(is_odd)
                        def _():
                            pl.semaphore_wait(bar, 1)
                        first = False

                    @pl.when(jnp.logical_or(jnp.logical_not(is_odd), b_e == b))
                    def _(b=b, c=c):
                        x_send(b, c).start()

        if not TAB_EARLY:
            tables_rest()

        if ASYM:
            @pl.when(is_odd)
            def _():
                pl.semaphore_wait(hs_sem, 1)
                for c in range(len(XCH)):
                    x_send(b_l, c).start()

        z = jnp.zeros((D, 128), bf16)
        for buf in (qT_own, qT_rem):
            for b in range(2):
                for h in range(H):
                    off = (1 - h % 2) * D
                    buf[b, h, off:off + D, :] = z

        def rope(t, c, s):
            if ROPE_GATHER:
                idx = jnp.bitwise_xor(lax.broadcasted_iota(jnp.int32, t.shape, 1), 1)
                sw = jnp.take_along_axis(t, idx, axis=1)
            else:
                ev = (lax.broadcasted_iota(jnp.int32, t.shape, 1) % 2) == 0
                sw = jnp.where(ev, pltpu.roll(t, 127, 1), pltpu.roll(t, 1, 1))
            return t * c + sw * s

        def xcat(src, b, q0, nq):
            return jnp.concatenate([src[b, q] for q in range(q0, q0 + nq)], axis=1)

        w_ld[0].wait()
        wqb[...] = wq32[...].astype(bf16)
        eye = (lax.broadcasted_iota(jnp.int32, (128, 128), 0)
               == lax.broadcasted_iota(jnp.int32, (128, 128), 1)).astype(bf16)
        qs = {}
        for b in (1, 0):
            qs[b] = _dot(xcat(xb, b, 0, 4), wqb[...])
        for b in (1, 0):
            for t in range(2):
                qt = rope(qs[b][:, t * 128:(t + 1) * 128], tabs[2], tabs[3]).astype(bf16)
                qtT = _dot(eye, qt, NT).astype(bf16)
                for hh in range(2):
                    h = 2 * t + hh
                    qT_own[b, h, hh * D:(hh + 1) * D, :] = qtT[hh * D:(hh + 1) * D]
        for h in range(H):
            for b in (1, 0):
                q_send(b, h).start()

        def kstore(b, k, dst0, ct, st):
            for t in range(2):
                kt = rope(k[:, t * 128:(t + 1) * 128], tabs[ct], tabs[st])
                kbuf[b, t, dst0:dst0 + R, :] = kt.astype(bf16)

        def vstore(b, v, dst0):
            vb = v.astype(bf16)
            for h in range(H):
                vT[b, h, :, dst0:dst0 + R] = vb[h * D:(h + 1) * D]

        w_ld[1].wait()
        wkb[...] = wk32[...].astype(bf16)
        ks = {b: _dot(xcat(xb, b, 0, 4), wkb[...]) for b in (1, 0)}
        for b in (1, 0):
            kstore(b, ks[b], 0, 0, 1)
        w_ld[2].wait()
        wvT[...] = wv32[...].T.astype(bf16)
        for b in (1, 0):
            vstore(b, _dot(wvT[...], xcat(xb, b, 0, 4), NT), 0)

        early = list(range(len(XCH) - NLATE))
        late = list(range(len(XCH) - NLATE, len(XCH)))
        qsplit = XCH[late[0]][0]
        KE = qsplit * 128

        def proj_kv(xs, k0, k1):
            nq = (k1 - k0) // 128
            nk = MSK.get(nq, 1)
            ck = R // nk
            kk = [_dot(xs[i * ck:(i + 1) * ck], wkb[k0:k1, :]) for i in range(nk)]
            kk = jnp.concatenate(kk, axis=0) if nk > 1 else kk[0]
            nv = MSV.get(nq, 1)
            c = HD // nv
            vs = [_dot(wvT[i * c:(i + 1) * c, k0:k1], xs, NT) for i in range(nv)]
            vv = jnp.concatenate(vs, axis=0) if nv > 1 else vs[0]
            return kk, vv

        def early_step(b):
            kk, vv = proj_kv(xcat(xr, b, 0, qsplit), 0, KE)
            kpart[b] = kk
            vpart[b] = vv

        def late_step(b):
            xl = xcat(xr, b, qsplit, 4 - qsplit)
            k2, v2 = proj_kv(xl, KE, DM)
            kstore(b, k2 + kpart[b], R, 4 + 2 * b, 5 + 2 * b)
            vstore(b, v2 + vpart[b], R)

        def wait_x(b, cs):
            for c in cs:
                x_send(b, c).wait_recv()

        def s_stage(b, h, qbuf):
            t = h // 2
            qp = qbuf[b, h]
            c = 2 * R // SS
            return [_dot(kbuf[b, t, i * c:(i + 1) * c, :], qp) for i in range(SS)]

        def sm_stage(parts):
            sT = jnp.concatenate(parts, axis=0) if len(parts) > 1 else parts[0]
            m = jnp.max(sT, axis=0, keepdims=True)
            p = jnp.exp2(sT - m)
            l = jnp.sum(p, axis=0, keepdims=True)
            return p.astype(bf16), m, l

        def pv_stage(b, h, pb_):
            c = D // SP
            os_ = [_dot(vT[b, h, i * c:(i + 1) * c, :], pb_) for i in range(SP)]
            return jnp.concatenate(os_, axis=0) if SP > 1 else os_[0]

        def foreign(units, pre=None):
            for (b, h) in units:
                q_send(b, h).wait_recv()
            if pre is not None:
                pre()
            parts = [s_stage(b, h, qT_rem) for (b, h) in units]
            res = []
            for (b, h), pt in zip(units, parts):
                pb_, m, l = sm_stage(pt)
                res.append((pv_stage(b, h, pb_), m, l))
            for (b, h), (oT, m, l) in zip(units, res):
                o_send[b, h, 0:32, :] = pltpu.bitcast(oT.astype(bf16), f32)
                o_send[b, h, 32:33, :] = m
                o_send[b, h, 33:34, :] = l
                o_send_cp(b, h).start()

        def own(units):
            parts = [s_stage(b, h, qT_own) for (b, h) in units]
            for (b, h), pt in zip(units, parts):
                pb_, m, l = sm_stage(pt)
                o_own[b, h] = pv_stage(b, h, pb_)
                st_own[b, h, 0:1, :] = m
                st_own[b, h, 1:2, :] = l

        def wo_cast():
            w_ld[3].wait()
            wob[...] = wo32[...].astype(bf16)

        @pl.when(is_odd)
        def _():
            bf_ = jnp.where(me == 1, 1, 0)
            bs_ = 1 - bf_
            wait_x(bs_, early)
            early_step(bs_)
            wait_x(bf_, early)
            early_step(bf_)
            wo_cast()
            if ODD_LATE_S_FIRST:
                wait_x(bs_, late)
                late_step(bs_)
            wait_x(bf_, late)
            units = [(bf_, h) for h in range(H)] + [(bs_, h) for h in range(H)]
            for gi, g in enumerate(ODD_GROUPS):
                pre = None
                if gi == 0:
                    if ODD_FUSE:
                        pre = lambda: late_step(bf_)
                    else:
                        late_step(bf_)
                if not ODD_LATE_S_FIRST and g[-1] >= 4 and all(gg[-1] < 4 for gg in ODD_GROUPS[:gi]):
                    wait_x(bs_, late)
                    late_step(bs_)
                foreign([units[u] for u in g], pre)

        @pl.when(jnp.logical_not(is_odd))
        def _():
            for b in (1, 0):
                wait_x(b, early)
            if EVEN_JOINT:
                kv = {b: proj_kv(xcat(xr, b, 0, qsplit), 0, KE) for b in (1, 0)}
                for b in (1, 0):
                    kpart[b] = kv[b][0]
                    vpart[b] = kv[b][1]
            else:
                for b in (1, 0):
                    early_step(b)
            wo_cast()
            for b in (1, 0):
                wait_x(b, late)
            if EVEN_JOINT:
                kv = {b: proj_kv(xcat(xr, b, qsplit, 4 - qsplit), KE, DM) for b in (1, 0)}
                for b in (1, 0):
                    kstore(b, kv[b][0] + kpart[b], R, 4 + 2 * b, 5 + 2 * b)
                for b in (1, 0):
                    vstore(b, kv[b][1] + vpart[b], R)
            else:
                for b in (1, 0):
                    late_step(b)
            units = [(1 - u % 2, u // 2) for u in range(8)]
            for g in EVEN_GROUPS:
                foreign([units[u] for u in g])

        own([(b, h) for h in range(H) for b in (1, 0)])

        for c in range(len(XCH)):
            for b in range(2):
                x_send(b, c).wait_send()
        for h in range(H):
            for b in range(2):
                q_send(b, h).wait_send()

        def merge(b, h):
            m1 = st_own[b, h, 0:1, :]
            l1 = st_own[b, h, 1:2, :]
            m2 = o_recv[b, h, 32:33, :]
            l2 = o_recv[b, h, 33:34, :]
            m = jnp.maximum(m1, m2)
            a1 = jnp.exp2(m1 - m)
            a2 = jnp.exp2(m2 - m)
            inv_l = 1.0 / (a1 * l1 + a2 * l2)
            o2 = pltpu.bitcast(o_recv[b, h, 0:32, :], bf16).astype(f32)
            c = o_own[b, h] * (a1 * inv_l) + o2 * (a2 * inv_l)
            ctxT[b, h * D:(h + 1) * D, :] = c.astype(bf16)

        for t in range(2):
            for hh in range(2):
                h = 2 * t + hh
                if h == H - 1:
                    for hp in range(H):
                        for b in range(2):
                            o_send_cp(b, hp).wait_send()
                for b in (1, 0):
                    o_send_cp(b, h).wait_recv()
                for b in (1, 0):
                    merge(b, h)
            for b in (1, 0):
                y = _dot(ctxT[b, t * 128:(t + 1) * 128, :], wob[t * 128:(t + 1) * 128, :], TN)
                if t == 0:
                    out_ref[b] = y
                else:
                    out_ref[b] = out_ref[b] + y

    return body


def make(cfg):
    nx = len(cfg.get("xch", XCH_DEFAULT))

    def kernel(x, Wq, Wk, Wv, Wo):
        V = pltpu.VMEM
        DMA = pltpu.SemaphoreType.DMA
        scratch = [
            V((2, R, DM), f32), V((DM, HD), f32), V((DM, HD), f32), V((DM, HD), f32), V((HD, DM), f32),
            V((2, 4, R, 128), bf16), V((2, 4, R, 128), bf16), V((DM, HD), bf16), V((DM, HD), bf16), V((HD, DM), bf16), V((HD, DM), bf16),
            V((2, H, 128, 128), bf16), V((2, H, 128, 128), bf16), V((2, 2, 2 * R, 128), bf16), V((2, H, D, 2 * R), bf16),
            V((2, H, D, R), f32), V((2, H, 8, 128), f32), V((2, H, 40, 128), f32), V((2, H, 40, 128), f32), V((2, HD, R), bf16),
            V((2, R, HD), f32), V((2, HD, R), f32),
            V((8, R, 128), f32),
            DMA((2 * nx + 4,)), DMA((2, nx)), DMA((2, nx)),
            DMA((2, H)), DMA((2, H)), DMA((2, H)), DMA((2, H)), pltpu.SemaphoreType.REGULAR,
        ]
        return pl.pallas_call(
            make_kernel(cfg),
            out_shape=jax.ShapeDtypeStruct((2, R, DM), f32),
            in_specs=[pl.BlockSpec(memory_space=pl.ANY)] * 5,
            out_specs=pl.BlockSpec(memory_space=pltpu.VMEM),
            scratch_shapes=scratch,
            compiler_params=pltpu.CompilerParams(collective_id=0, vmem_limit_bytes=64 * 1024 * 1024,
                                                 disable_semaphore_checks=cfg.get("nosemcheck", True),
                                                 disable_bounds_checks=cfg.get("nobounds", False),
                                                 fuse_transposed_lhs_in_matmul=cfg.get("fuse_tl", False)),
        )(x, Wq, Wk, Wv, Wo)
    return kernel

kernel = make({})


def pallas_dist_rope_attn_qseq_b2_sq128_d512_hq4_dh64_kernel(
    x: jax.Array,
    Wq: jax.Array,
    Wk: jax.Array,
    Wv: jax.Array,
    Wo: jax.Array,
):
    return kernel(x, Wq, Wk, Wv, Wo)
```

```python
import numpy as np
import jax
import jax.numpy as jnp
from jax import lax
from jax.experimental import pallas as pl
from jax.experimental.pallas import tpu as pltpu

f32 = jnp.float32
bf16 = jnp.bfloat16
NT = (((1,), (1,)), ((), ()))
TN = (((0,), (0,)), ((), ()))
MESH = pl.DeviceIdType.MESH

R = 128
DM = 512
H = 4
D = 64
HD = H * D
QSCALE = float(0.125 * np.log2(np.e))
LN_BASE = float(np.log(10000.0))

XCH = ((0, 1, 0, 64), (0, 1, 64, 64), (1, 2, 0, 128), (3, 1, 0, 128))
EARLY = (0, 1, 2)
LATE = (3,)
KE = 384
OROWS = 33


def _dot(a, b, dims=None):
    if dims is None:
        return jnp.dot(a, b, preferred_element_type=f32)
    return lax.dot_general(a, b, dims, preferred_element_type=f32)


def _body(x_hbm, wq_hbm, wk_hbm, wv_hbm, wo_hbm, out_ref,
          xf, wq32, wk32, wv32, wo32,
          xb, xr, wkb, wvT, wob,
          qT_own, qT_rem, kbuf, vT,
          o_own, st_own, o_send, o_recv, ctxT,
          kpart, vpart, tabs,
          ld_sem, xs_sem, xr_sem, qs_sem, qr_sem, os_sem, or_sem, hs_sem):
    me = lax.axis_index("i")
    pa = jnp.bitwise_xor(me, 1)
    pb = 3 - me
    is_odd = (me % 2) == 1

    def kv_partner(b):
        return (pa, pb)[b] if isinstance(b, int) else jnp.where(b == 0, pa, pb)

    def q_partner(b):
        return (pb, pa)[b] if isinstance(b, int) else jnp.where(b == 0, pb, pa)

    def x_load(b, c, n):
        q0, nq, r0, nr = XCH[c]
        return pltpu.make_async_copy(
            x_hbm.at[b, pl.ds(r0, nr), pl.ds(q0 * 128, nq * 128)],
            xf.at[b, pl.ds(r0, nr), pl.ds(q0 * 128, nq * 128)], ld_sem.at[n])

    def x_send(b, c):
        q0, nq, r0, nr = XCH[c]
        return pltpu.make_async_remote_copy(
            xb.at[b, pl.ds(q0, nq), pl.ds(r0, nr)], xr.at[b, pl.ds(q0, nq), pl.ds(r0, nr)],
            xs_sem.at[b, c], xr_sem.at[b, c], device_id=(kv_partner(b),), device_id_type=MESH)

    def q_send(b, h):
        if isinstance(h, int):
            rows = pl.ds((h % 2) * D, D)
        else:
            rows = pl.ds(pl.multiple_of((h % 2) * D, D), D)
        return pltpu.make_async_remote_copy(
            qT_own.at[b, h, rows], qT_rem.at[b, h, rows],
            qs_sem.at[b, h], qr_sem.at[b, h], device_id=(q_partner(b),), device_id_type=MESH)

    def o_copy(b, h):
        return pltpu.make_async_remote_copy(
            o_send.at[b, h, pl.ds(0, OROWS)], o_recv.at[b, h, pl.ds(0, OROWS)],
            os_sem.at[b, h], or_sem.at[b, h], device_id=(q_partner(b),), device_id_type=MESH)

    nx = len(XCH)
    for c in range(nx):
        for b in range(2):
            x_load(b, c, 2 * c + b).start()

    bar = pltpu.get_barrier_semaphore()

    @pl.when(me != 2)
    def _():
        pl.semaphore_signal(bar, inc=1, device_id=(pa,), device_id_type=MESH)
        pl.semaphore_signal(bar, inc=1, device_id=(pb,), device_id_type=MESH)

    w_loads = []
    for n, (src, dst) in enumerate(((wq_hbm, wq32), (wk_hbm, wk32), (wv_hbm, wv32), (wo_hbm, wo32))):
        cp = pltpu.make_async_copy(src, dst, ld_sem.at[2 * nx + n])
        cp.start()
        w_loads.append(cp)

    @pl.when(me == 2)
    def _():
        pl.semaphore_wait(bar, 2)
        pl.semaphore_signal(hs_sem, inc=1, device_id=(pa,), device_id_type=MESH)
        pl.semaphore_signal(hs_sem, inc=1, device_id=(pb,), device_id_type=MESH)

    r16 = lax.broadcasted_iota(jnp.int32, (16, 128), 0)
    l16 = lax.broadcasted_iota(jnp.int32, (16, 128), 1)
    inv16 = jnp.exp(((l16 % D) // 2).astype(f32) * (-2.0 / D * LN_BASE))
    pos16 = jnp.where(r16 < 8, r16 + me * R,
            jnp.where(r16 == 8, 8,
            jnp.where(r16 == 9, 16,
            jnp.where(r16 == 10, 32,
            jnp.where(r16 == 11, 64,
            jnp.where(r16 == 12, (pa - me) * R, (pb - me) * R))))))
    ang16 = pos16.astype(f32) * inv16
    c16 = jnp.cos(ang16)
    s16 = jnp.sin(ang16)

    def rot(c, s, row):
        cd = c16[row:row + 1]
        sd = s16[row:row + 1]
        return c * cd - s * sd, s * cd + c * sd

    c_own, s_own = c16[0:8], s16[0:8]
    for k in range(4):
        c2, s2 = rot(c_own, s_own, 8 + k)
        c_own = jnp.concatenate([c_own, c2], axis=0)
        s_own = jnp.concatenate([s_own, s2], axis=0)
    lane = lax.broadcasted_iota(jnp.int32, (R, 128), 1)
    sgn = jnp.where((lane % 2) == 0, -1.0, 1.0).astype(f32)
    tabs[0] = c_own
    tabs[1] = s_own * sgn
    tabs[2] = c_own * QSCALE
    tabs[3] = s_own * sgn * QSCALE
    for b in range(2):
        cb, sb = rot(c_own, s_own, 12 + b)
        tabs[4 + 2 * b] = cb
        tabs[5 + 2 * b] = sb * sgn

    def rope(t, c, s):
        idx = jnp.bitwise_xor(lax.broadcasted_iota(jnp.int32, t.shape, 1), 1)
        return t * c + jnp.take_along_axis(t, idx, axis=1) * s

    b_l = jnp.where(me == 1, 1, 0)
    b_e = 1 - b_l
    for c, (q0, nq, r0, nr) in enumerate(XCH):
        for b in range(2):
            x_load(b, c, 2 * c + b).wait()
            for q in range(q0, q0 + nq):
                xb[b, q, r0:r0 + nr, :] = xf[b, r0:r0 + nr, q * 128:(q + 1) * 128].astype(bf16)
            if c == 0 and b == 0:
                @pl.when(me == 0)
                def _():
                    pl.semaphore_wait(bar, 2)

                @pl.when(is_odd)
                def _():
                    pl.semaphore_wait(bar, 1)

            @pl.when(jnp.logical_or(jnp.logical_not(is_odd), b_e == b))
            def _(b=b, c=c):
                x_send(b, c).start()

    @pl.when(is_odd)
    def _():
        pl.semaphore_wait(hs_sem, 1)
        for c in range(nx):
            x_send(b_l, c).start()

    zeros = jnp.zeros((D, 128), bf16)
    for buf in (qT_own, qT_rem):
        for b in range(2):
            for h in range(H):
                off = (1 - h % 2) * D
                buf[b, h, off:off + D, :] = zeros

    def xcat(src, b, q0, nq):
        return jnp.concatenate([src[b, q] for q in range(q0, q0 + nq)], axis=1)

    w_loads[0].wait()
    wq = wq32[...].astype(bf16)
    eye = (lax.broadcasted_iota(jnp.int32, (128, 128), 0)
           == lax.broadcasted_iota(jnp.int32, (128, 128), 1)).astype(bf16)
    qs = {b: _dot(xcat(xb, b, 0, 4), wq) for b in (1, 0)}
    for b in (1, 0):
        for t in range(2):
            qt = rope(qs[b][:, t * 128:(t + 1) * 128], tabs[2], tabs[3]).astype(bf16)
            qtT = _dot(eye, qt, NT).astype(bf16)
            for hh in range(2):
                qT_own[b, 2 * t + hh, hh * D:(hh + 1) * D, :] = qtT[hh * D:(hh + 1) * D]
    for h in range(H):
        for b in (1, 0):
            q_send(b, h).start()

    def kstore(b, k, row0, ct, st):
        for t in range(2):
            kt = rope(k[:, t * 128:(t + 1) * 128], tabs[ct], tabs[st])
            kbuf[b, t, row0:row0 + R, :] = kt.astype(bf16)

    def vstore(b, v, col0):
        vb = v.astype(bf16)
        for h in range(H):
            vT[b, h, :, col0:col0 + R] = vb[h * D:(h + 1) * D]

    w_loads[1].wait()
    wkb[...] = wk32[...].astype(bf16)
    ks = {b: _dot(xcat(xb, b, 0, 4), wkb[...]) for b in (1, 0)}
    for b in (1, 0):
        kstore(b, ks[b], 0, 0, 1)
    w_loads[2].wait()
    wvT[...] = wv32[...].T.astype(bf16)
    for b in (1, 0):
        vstore(b, _dot(wvT[...], xcat(xb, b, 0, 4), NT), 0)

    def proj_kv(xs, k0, k1):
        kk = jnp.concatenate([_dot(xs[i * 64:(i + 1) * 64], wkb[k0:k1, :]) for i in range(2)], axis=0)
        vv = jnp.concatenate([_dot(wvT[i * 64:(i + 1) * 64, k0:k1], xs, NT) for i in range(4)], axis=0)
        return kk, vv

    def early_kv(b):
        return proj_kv(xcat(xr, b, 0, 3), 0, KE)

    def late_kv(b):
        return proj_kv(xr[b, 3], KE, DM)

    def early_store(b, kv):
        kpart[b] = kv[0]
        vpart[b] = kv[1]

    def late_store_k(b, kv):
        kstore(b, kv[0] + kpart[b], R, 4 + 2 * b, 5 + 2 * b)

    def late_store_v(b, kv):
        vstore(b, kv[1] + vpart[b], R)

    def late_step(b):
        kv = late_kv(b)
        late_store_k(b, kv)
        late_store_v(b, kv)

    def wait_x(b, chunks):
        for c in chunks:
            x_send(b, c).wait_recv()

    def wo_cast():
        w_loads[3].wait()
        wob[...] = wo32[...].astype(bf16)

    def scores(b, h, qbuf):
        qp = qbuf[b, h]
        return [_dot(kbuf[b, h // 2, i * 64:(i + 1) * 64, :], qp) for i in range(4)]

    def softmax_pv(b, h, parts):
        sT = jnp.concatenate(parts, axis=0)
        m = jnp.max(sT, axis=0, keepdims=True)
        p = jnp.exp2(sT - m)
        l = jnp.sum(p, axis=0, keepdims=True)
        pb_ = p.astype(bf16)
        oT = jnp.concatenate([_dot(vT[b, h, i * 32:(i + 1) * 32, :], pb_) for i in range(2)], axis=0)
        return oT, m, l

    def foreign(units, pre=None):
        for b, h in units:
            q_send(b, h).wait_recv()
        if pre is not None:
            pre()
        parts = [scores(b, h, qT_rem) for b, h in units]
        res = [softmax_pv(b, h, pt) for (b, h), pt in zip(units, parts)]
        for (b, h), (oT, m, l) in zip(units, res):
            o_send[b, h, 0:32, :] = pltpu.bitcast((oT * (1.0 / l)).astype(bf16), f32)
            o_send[b, h, 32:33, :] = m + jnp.log2(l)
            o_copy(b, h).start()

    def own(units):
        parts = [scores(b, h, qT_own) for b, h in units]
        for (b, h), pt in zip(units, parts):
            oT, m, l = softmax_pv(b, h, pt)
            o_own[b, h] = oT
            st_own[b, h, 0:1, :] = m
            st_own[b, h, 1:2, :] = l

    @pl.when(is_odd)
    def _():
        bf_ = jnp.where(me == 1, 1, 0)
        bs_ = 1 - bf_
        wait_x(bs_, EARLY)
        early_store(bs_, early_kv(bs_))
        wait_x(bf_, EARLY)
        early_store(bf_, early_kv(bf_))
        wait_x(bf_, LATE)
        foreign([(bf_, 0)], lambda: late_step(bf_))
        for h in range(1, H):
            foreign([(bf_, h)])
        wait_x(bs_, LATE)
        late_step(bs_)
        foreign([(bs_, 0), (bs_, 1)])
        foreign([(bs_, 2), (bs_, 3)])
        wo_cast()

    @pl.when(jnp.logical_not(is_odd))
    def _():
        for b in (1, 0):
            wait_x(b, EARLY)
        kv = {b: early_kv(b) for b in (1, 0)}
        for b in (1, 0):
            early_store(b, kv[b])
        wo_cast()
        for b in (1, 0):
            wait_x(b, LATE)
        kv = {b: late_kv(b) for b in (1, 0)}
        for b in (1, 0):
            late_store_k(b, kv[b])
        for b in (1, 0):
            late_store_v(b, kv[b])
        for h in range(H):
            foreign([(1, h), (0, h)])

    own([(b, h) for h in range(H) for b in (1, 0)])

    for c in range(nx):
        for b in range(2):
            x_send(b, c).wait_send()
    for h in range(H):
        for b in range(2):
            q_send(b, h).wait_send()

    def merge(b, h):
        m1 = st_own[b, h, 0:1, :]
        l1 = st_own[b, h, 1:2, :]
        lse2 = o_recv[b, h, 32:33, :]
        o2 = pltpu.bitcast(o_recv[b, h, 0:32, :], bf16).astype(f32)
        m = jnp.maximum(m1, lse2)
        a1 = jnp.exp2(m1 - m)
        a2 = jnp.exp2(lse2 - m)
        inv_l = 1.0 / (a1 * l1 + a2)
        ctx = o_own[b, h] * (a1 * inv_l) + o2 * (a2 * inv_l)
        ctxT[b, h * D:(h + 1) * D, :] = ctx.astype(bf16)

    for t in range(2):
        for h in (2 * t, 2 * t + 1):
            if h == H - 1:
                for hp in range(H):
                    for b in range(2):
                        o_copy(b, hp).wait_send()
            for b in (1, 0):
                o_copy(b, h).wait_recv()
            for b in (1, 0):
                merge(b, h)
        for b in (1, 0):
            y = _dot(ctxT[b, t * 128:(t + 1) * 128, :], wob[t * 128:(t + 1) * 128, :], TN)
            out_ref[b] = y if t == 0 else out_ref[b] + y


def pallas_dist_rope_attn_qseq_b2_sq128_d512_hq4_dh64_kernel(
    x: jax.Array,
    Wq: jax.Array,
    Wk: jax.Array,
    Wv: jax.Array,
    Wo: jax.Array,
):
    V = pltpu.VMEM
    DMA = pltpu.SemaphoreType.DMA
    nx = len(XCH)
    scratch = [
        V((2, R, DM), f32), V((DM, HD), f32), V((DM, HD), f32), V((DM, HD), f32), V((HD, DM), f32),
        V((2, 4, R, 128), bf16), V((2, 4, R, 128), bf16), V((DM, HD), bf16), V((HD, DM), bf16), V((HD, DM), bf16),
        V((2, H, 128, 128), bf16), V((2, H, 128, 128), bf16), V((2, 2, 2 * R, 128), bf16), V((2, H, D, 2 * R), bf16),
        V((2, H, D, R), f32), V((2, H, 8, 128), f32), V((2, H, 40, 128), f32), V((2, H, 40, 128), f32), V((2, HD, R), bf16),
        V((2, R, HD), f32), V((2, HD, R), f32), V((8, R, 128), f32),
        DMA((2 * nx + 4,)), DMA((2, nx)), DMA((2, nx)),
        DMA((2, H)), DMA((2, H)), DMA((2, H)), DMA((2, H)), pltpu.SemaphoreType.REGULAR,
    ]
    return pl.pallas_call(
        _body,
        out_shape=jax.ShapeDtypeStruct((2, R, DM), f32),
        in_specs=[pl.BlockSpec(memory_space=pl.ANY)] * 5,
        out_specs=pl.BlockSpec(memory_space=pltpu.VMEM),
        scratch_shapes=scratch,
        compiler_params=pltpu.CompilerParams(
            collective_id=0,
            vmem_limit_bytes=64 * 1024 * 1024,
            disable_semaphore_checks=True,
            flags={"XLA_TPU_FORCE_LP_LLO_SCHEDULER": True},
        ),
    )(x, Wq, Wk, Wv, Wo)
```

```python
import numpy as np
import jax
import jax.numpy as jnp
from jax import lax
from jax.experimental import pallas as pl
from jax.experimental.pallas import tpu as pltpu

f32 = jnp.float32
bf16 = jnp.bfloat16
NT = (((1,), (1,)), ((), ()))
TN = (((0,), (0,)), ((), ()))
MESH = pl.DeviceIdType.MESH

R = 128
DM = 512
H = 4
D = 64
HD = H * D
QSCALE = float(0.125 * np.log2(np.e))
LN_BASE = float(np.log(10000.0))

XCH = ((0, 1, 0, 64), (0, 1, 64, 64), (1, 2, 0, 128), (3, 1, 0, 128))
EARLY = (0, 1, 2)
LATE = (3,)
KE = 384
OROWS = 33


def _dot(a, b, dims=None):
    if dims is None:
        return jnp.dot(a, b, preferred_element_type=f32)
    return lax.dot_general(a, b, dims, preferred_element_type=f32)


def _body(x_hbm, wq_hbm, wk_hbm, wv_hbm, wo_hbm, out_ref,
          xf, wq32, wk32, wv32, wo32,
          xb, xr, wkb, wvT, wob,
          qT_own, qT_rem, kbuf, vT,
          o_own, st_own, o_send, o_recv, ctxT,
          kpart, vpart, tabs,
          ld_sem, xs_sem, xr_sem, qs_sem, qr_sem, os_sem, or_sem, hs_sem):
    me = lax.axis_index("i")
    pa = jnp.bitwise_xor(me, 1)
    pb = 3 - me
    is_odd = (me % 2) == 1

    def kv_partner(b):
        return (pa, pb)[b] if isinstance(b, int) else jnp.where(b == 0, pa, pb)

    def q_partner(b):
        return (pb, pa)[b] if isinstance(b, int) else jnp.where(b == 0, pb, pa)

    def x_load(b, c, n):
        q0, nq, r0, nr = XCH[c]
        return pltpu.make_async_copy(
            x_hbm.at[b, pl.ds(r0, nr), pl.ds(q0 * 128, nq * 128)],
            xf.at[b, pl.ds(r0, nr), pl.ds(q0 * 128, nq * 128)], ld_sem.at[n])

    def x_send(b, c):
        q0, nq, r0, nr = XCH[c]
        return pltpu.make_async_remote_copy(
            xb.at[b, pl.ds(q0, nq), pl.ds(r0, nr)], xr.at[b, pl.ds(q0, nq), pl.ds(r0, nr)],
            xs_sem.at[b, c], xr_sem.at[b, c], device_id=(kv_partner(b),), device_id_type=MESH)

    def q_send(b, h):
        rows = pl.ds((h % 2) * D, D)
        return pltpu.make_async_remote_copy(
            qT_own.at[b, h, rows], qT_rem.at[b, h, rows],
            qs_sem.at[b, h], qr_sem.at[b, h], device_id=(q_partner(b),), device_id_type=MESH)

    def o_copy(b, h):
        return pltpu.make_async_remote_copy(
            o_send.at[b, h, pl.ds(0, OROWS)], o_recv.at[b, h, pl.ds(0, OROWS)],
            os_sem.at[b, h], or_sem.at[b, h], device_id=(q_partner(b),), device_id_type=MESH)

    nx = len(XCH)
    for c in range(nx):
        for b in range(2):
            x_load(b, c, 2 * c + b).start()

    bar = pltpu.get_barrier_semaphore()

    @pl.when(me != 2)
    def _():
        pl.semaphore_signal(bar, inc=1, device_id=(pa,), device_id_type=MESH)
        pl.semaphore_signal(bar, inc=1, device_id=(pb,), device_id_type=MESH)

    w_loads = []
    for n, (src, dst) in enumerate(((wq_hbm, wq32), (wk_hbm, wk32), (wv_hbm, wv32), (wo_hbm, wo32))):
        cp = pltpu.make_async_copy(src, dst, ld_sem.at[2 * nx + n])
        cp.start()
        w_loads.append(cp)

    @pl.when(me == 2)
    def _():
        pl.semaphore_wait(bar, 2)
        pl.semaphore_signal(hs_sem, inc=1, device_id=(pa,), device_id_type=MESH)
        pl.semaphore_signal(hs_sem, inc=1, device_id=(pb,), device_id_type=MESH)

    r16 = lax.broadcasted_iota(jnp.int32, (16, 128), 0)
    l16 = lax.broadcasted_iota(jnp.int32, (16, 128), 1)
    inv16 = jnp.exp(((l16 % D) // 2).astype(f32) * (-2.0 / D * LN_BASE))
    pos16 = jnp.where(r16 < 8, r16 + me * R,
            jnp.where(r16 == 8, 8,
            jnp.where(r16 == 9, 16,
            jnp.where(r16 == 10, 32,
            jnp.where(r16 == 11, 64,
            jnp.where(r16 == 12, (pa - me) * R, (pb - me) * R))))))
    ang16 = pos16.astype(f32) * inv16
    c16 = jnp.cos(ang16)
    s16 = jnp.sin(ang16)

    def rot(c, s, row):
        cd = c16[row:row + 1]
        sd = s16[row:row + 1]
        return c * cd - s * sd, s * cd + c * sd

    c_own, s_own = c16[0:8], s16[0:8]
    for k in range(4):
        c2, s2 = rot(c_own, s_own, 8 + k)
        c_own = jnp.concatenate([c_own, c2], axis=0)
        s_own = jnp.concatenate([s_own, s2], axis=0)
    lane = lax.broadcasted_iota(jnp.int32, (R, 128), 1)
    sgn = jnp.where((lane % 2) == 0, -1.0, 1.0).astype(f32)
    tabs[0] = c_own
    tabs[1] = s_own * sgn
    tabs[2] = c_own * QSCALE
    tabs[3] = s_own * sgn * QSCALE
    for b in range(2):
        cb, sb = rot(c_own, s_own, 12 + b)
        tabs[4 + 2 * b] = cb
        tabs[5 + 2 * b] = sb * sgn

    def rope(t, c, s):
        even = (lax.broadcasted_iota(jnp.int32, t.shape, 1) % 2) == 0
        return t * c + jnp.where(even, pltpu.roll(t, 127, 1), pltpu.roll(t, 1, 1)) * s

    b_l = jnp.where(me == 1, 1, 0)
    b_e = 1 - b_l
    for c, (q0, nq, r0, nr) in enumerate(XCH):
        for b in range(2):
            x_load(b, c, 2 * c + b).wait()
            for q in range(q0, q0 + nq):
                xb[b, q, r0:r0 + nr, :] = xf[b, r0:r0 + nr, q * 128:(q + 1) * 128].astype(bf16)
            if c == 0 and b == 0:
                @pl.when(me == 0)
                def _():
                    pl.semaphore_wait(bar, 2)

                @pl.when(is_odd)
                def _():
                    pl.semaphore_wait(bar, 1)

            @pl.when(jnp.logical_or(jnp.logical_not(is_odd), b_e == b))
            def _(b=b, c=c):
                x_send(b, c).start()

    @pl.when(is_odd)
    def _():
        pl.semaphore_wait(hs_sem, 1)
        for c in range(nx):
            x_send(b_l, c).start()

    zeros = jnp.zeros((D, 128), bf16)
    for buf in (qT_own, qT_rem):
        for b in range(2):
            for h in range(H):
                off = (1 - h % 2) * D
                buf[b, h, off:off + D, :] = zeros

    def xcat(src, b, q0, nq):
        return jnp.concatenate([src[b, q] for q in range(q0, q0 + nq)], axis=1)

    w_loads[0].wait()
    wq = wq32[...].astype(bf16)
    eye = (lax.broadcasted_iota(jnp.int32, (128, 128), 0)
           == lax.broadcasted_iota(jnp.int32, (128, 128), 1)).astype(bf16)
    qs = {b: _dot(xcat(xb, b, 0, 4), wq) for b in (1, 0)}
    for b in (1, 0):
        for t in range(2):
            qt = rope(qs[b][:, t * 128:(t + 1) * 128], tabs[2], tabs[3]).astype(bf16)
            qtT = _dot(eye, qt, NT).astype(bf16)
            for hh in range(2):
                qT_own[b, 2 * t + hh, hh * D:(hh + 1) * D, :] = qtT[hh * D:(hh + 1) * D]
    for h in range(H):
        for b in (1, 0):
            q_send(b, h).start()

    def kstore(b, k, row0, ct, st):
        for t in range(2):
            kt = rope(k[:, t * 128:(t + 1) * 128], tabs[ct], tabs[st])
            kbuf[b, t, row0:row0 + R, :] = kt.astype(bf16)

    def vstore(b, v, col0):
        vb = v.astype(bf16)
        for h in range(H):
            vT[b, h, :, col0:col0 + R] = vb[h * D:(h + 1) * D]

    w_loads[1].wait()
    wkb[...] = wk32[...].astype(bf16)
    ks = {b: _dot(xcat(xb, b, 0, 4), wkb[...]) for b in (1, 0)}
    for b in (1, 0):
        kstore(b, ks[b], 0, 0, 1)
    w_loads[2].wait()
    wvT[...] = wv32[...].T.astype(bf16)
    for b in (1, 0):
        vstore(b, _dot(wvT[...], xcat(xb, b, 0, 4), NT), 0)

    def proj_kv(xs, k0, k1):
        kk = jnp.concatenate([_dot(xs[i * 64:(i + 1) * 64], wkb[k0:k1, :]) for i in range(2)], axis=0)
        vv = jnp.concatenate([_dot(wvT[i * 64:(i + 1) * 64, k0:k1], xs, NT) for i in range(4)], axis=0)
        return kk, vv

    def early_kv(b):
        return proj_kv(xcat(xr, b, 0, 3), 0, KE)

    def late_kv(b):
        return proj_kv(xr[b, 3], KE, DM)

    def early_store(b, kv):
        kpart[b] = kv[0]
        vpart[b] = kv[1]

    def late_store_k(b, kv):
        kstore(b, kv[0] + kpart[b], R, 4 + 2 * b, 5 + 2 * b)

    def late_store_v(b, kv):
        vstore(b, kv[1] + vpart[b], R)

    def late_step(b):
        kv = late_kv(b)
        late_store_k(b, kv)
        late_store_v(b, kv)

    def wait_x(b, chunks):
        for c in chunks:
            x_send(b, c).wait_recv()

    def wo_cast():
        w_loads[3].wait()
        wob[...] = wo32[...].astype(bf16)

    def scores(b, h, qbuf):
        qp = qbuf[b, h]
        return [_dot(kbuf[b, h // 2, i * 64:(i + 1) * 64, :], qp) for i in range(4)]

    def softmax_pv(b, h, parts):
        sT = jnp.concatenate(parts, axis=0)
        m = jnp.max(sT, axis=0, keepdims=True)
        p = jnp.exp2(sT - m)
        l = jnp.sum(p, axis=0, keepdims=True)
        pb_ = p.astype(bf16)
        oT = jnp.concatenate([_dot(vT[b, h, i * 32:(i + 1) * 32, :], pb_) for i in range(2)], axis=0)
        return oT, m, l

    def foreign(units, pre=None):
        for b, h in units:
            q_send(b, h).wait_recv()
        if pre is not None:
            pre()
        parts = [scores(b, h, qT_rem) for b, h in units]
        res = [softmax_pv(b, h, pt) for (b, h), pt in zip(units, parts)]
        for (b, h), (oT, m, l) in zip(units, res):
            o_send[b, h, 0:32, :] = pltpu.bitcast((oT * (1.0 / l)).astype(bf16), f32)
            o_send[b, h, 32:33, :] = m + jnp.log2(l)
            o_copy(b, h).start()

    def own(units):
        parts = [scores(b, h, qT_own) for b, h in units]
        for (b, h), pt in zip(units, parts):
            oT, m, l = softmax_pv(b, h, pt)
            o_own[b, h] = oT
            st_own[b, h, 0:1, :] = m
            st_own[b, h, 1:2, :] = l

    @pl.when(is_odd)
    def _():
        bf_ = jnp.where(me == 1, 1, 0)
        bs_ = 1 - bf_
        wait_x(bs_, EARLY)
        early_store(bs_, early_kv(bs_))
        wait_x(bf_, EARLY)
        early_store(bf_, early_kv(bf_))
        wait_x(bf_, LATE)
        foreign([(bf_, 0)], lambda: late_step(bf_))
        for h in range(1, H):
            foreign([(bf_, h)])
        wait_x(bs_, LATE)
        late_step(bs_)
        foreign([(bs_, 0), (bs_, 1)])
        foreign([(bs_, 2), (bs_, 3)])
        wo_cast()

    @pl.when(jnp.logical_not(is_odd))
    def _():
        for b in (1, 0):
            wait_x(b, EARLY)
        kv = {b: early_kv(b) for b in (1, 0)}
        for b in (1, 0):
            early_store(b, kv[b])
        wo_cast()
        for b in (1, 0):
            wait_x(b, LATE)
        kv = {b: late_kv(b) for b in (1, 0)}
        for b in (1, 0):
            late_store_k(b, kv[b])
        for b in (1, 0):
            late_store_v(b, kv[b])
        for h in range(H):
            foreign([(1, h), (0, h)])

    own([(b, h) for h in range(H) for b in (1, 0)])

    for c in range(nx):
        for b in range(2):
            x_send(b, c).wait_send()
    for h in range(H):
        for b in range(2):
            q_send(b, h).wait_send()

    def merge(b, h):
        m1 = st_own[b, h, 0:1, :]
        l1 = st_own[b, h, 1:2, :]
        lse2 = o_recv[b, h, 32:33, :]
        o2 = pltpu.bitcast(o_recv[b, h, 0:32, :], bf16).astype(f32)
        m = jnp.maximum(m1, lse2)
        a1 = jnp.exp2(m1 - m)
        a2 = jnp.exp2(lse2 - m)
        inv_l = 1.0 / (a1 * l1 + a2)
        ctx = o_own[b, h] * (a1 * inv_l) + o2 * (a2 * inv_l)
        ctxT[b, h * D:(h + 1) * D, :] = ctx.astype(bf16)

    for t in range(2):
        for h in (2 * t, 2 * t + 1):
            if h == H - 1:
                for hp in range(H):
                    for b in range(2):
                        o_copy(b, hp).wait_send()
            for b in (1, 0):
                o_copy(b, h).wait_recv()
            for b in (1, 0):
                merge(b, h)
        for b in (1, 0):
            y = _dot(ctxT[b, t * 128:(t + 1) * 128, :], wob[t * 128:(t + 1) * 128, :], TN)
            out_ref[b] = y if t == 0 else out_ref[b] + y


def pallas_dist_rope_attn_qseq_b2_sq128_d512_hq4_dh64_kernel(
    x: jax.Array,
    Wq: jax.Array,
    Wk: jax.Array,
    Wv: jax.Array,
    Wo: jax.Array,
):
    V = pltpu.VMEM
    DMA = pltpu.SemaphoreType.DMA
    nx = len(XCH)
    scratch = [
        V((2, R, DM), f32), V((DM, HD), f32), V((DM, HD), f32), V((DM, HD), f32), V((HD, DM), f32),
        V((2, 4, R, 128), bf16), V((2, 4, R, 128), bf16), V((DM, HD), bf16), V((HD, DM), bf16), V((HD, DM), bf16),
        V((2, H, 128, 128), bf16), V((2, H, 128, 128), bf16), V((2, 2, 2 * R, 128), bf16), V((2, H, D, 2 * R), bf16),
        V((2, H, D, R), f32), V((2, H, 8, 128), f32), V((2, H, 40, 128), f32), V((2, H, 40, 128), f32), V((2, HD, R), bf16),
        V((2, R, HD), f32), V((2, HD, R), f32), V((8, R, 128), f32),
        DMA((2 * nx + 4,)), DMA((2, nx)), DMA((2, nx)),
        DMA((2, H)), DMA((2, H)), DMA((2, H)), DMA((2, H)), pltpu.SemaphoreType.REGULAR,
    ]
    return pl.pallas_call(
        _body,
        out_shape=jax.ShapeDtypeStruct((2, R, DM), f32),
        in_specs=[pl.BlockSpec(memory_space=pl.ANY)] * 5,
        out_specs=pl.BlockSpec(memory_space=pltpu.VMEM),
        scratch_shapes=scratch,
        compiler_params=pltpu.CompilerParams(
            collective_id=0,
            vmem_limit_bytes=64 * 1024 * 1024,
            disable_semaphore_checks=True,
            flags={"XLA_TPU_FORCE_LP_LLO_SCHEDULER": True},
        ),
    )(x, Wq, Wk, Wv, Wo)
```
